```python
import numpy as np

kernel_name = "dist_layernorm_xy_m6144_n2048"

def setup_inputs():
    x = np.random.randn(12288, 4096).astype(np.float32)
    gamma = np.random.randn(4096).astype(np.float32)
    beta = np.random.randn(4096).astype(np.float32)
    return {"x": x, "gamma": gamma, "beta": beta}

def reference(x: np.ndarray, gamma: np.ndarray, beta: np.ndarray) -> np.ndarray:
    eps = 1e-5
    mean = np.mean(x, axis=1, keepdims=True)
    var = np.var(x, axis=1, keepdims=True)
    return gamma * (x - mean) / np.sqrt(var + eps) + beta
```

```python
import numpy as np

import jax
import jax.numpy as jnp
from jax import lax
from jax.experimental import pallas as pl
from jax.experimental.pallas import tpu as pltpu

_EPS = 1e-5
_Y_SIZE = 2
_BIG = 1024
_TAIL = (512, 256, 128, 96, 32)
_NORM_AFTER = ((), (0,), (), (), (1, 2, 3, 4))
_TILE = 512
_UNIT = 256
_SUB = 64
_DIRECT_MAX = 32


def _make_body(M, N, n_big):
    n_tail = len(_TAIL)
    n_total = _Y_SIZE * N
    tail_row = [n_big * _BIG + int(s) for s in np.cumsum((0,) + _TAIL[:-1])]
    big_tiles = _BIG // _TILE
    tail_tiles = [-(-r // _TILE) for r in _TAIL]
    tail_tile0 = [n_big * big_tiles + int(s) for s in np.cumsum([0] + tail_tiles[:-1])]
    n_tiles = n_big * big_tiles + sum(tail_tiles)
    late = list(_NORM_AFTER[-1])
    early = [t for t in range(n_tail) if t not in late]
    assert sorted(early + late) == sorted(sum(map(list, _NORM_AFTER), []))

    def body(x_hbm, g_hbm, b_hbm, o_ref,
             xbuf, gbuf, bbuf, gb8, sbuf, rbuf, send_sem, late_sems):
        nbr = (lax.axis_index("x"), 1 - lax.axis_index("y"))

        def stat_copy(tile0, tiles, recv_sem):
            return pltpu.make_async_remote_copy(
                src_ref=sbuf.at[pl.ds(tile0, tiles)], dst_ref=rbuf.at[pl.ds(tile0, tiles)],
                send_sem=send_sem, recv_sem=recv_sem,
                device_id=nbr, device_id_type=pl.DeviceIdType.MESH)

        def lanes():
            return lax.broadcasted_iota(jnp.int32, (8, 128), 1)

        def stats_unit(row0, rows, lane, tile):
            for o in range(0, rows, _SUB):
                sub = min(_SUB, rows - o)
                r0 = pl.multiple_of(row0 + o, 8)
                mean = jnp.sum(xbuf[pl.ds(r0, sub), :], axis=1, keepdims=True) * (1.0 / N)
                d = xbuf[pl.ds(r0, sub), :] - mean
                m2 = jnp.sum(d * d, axis=1, keepdims=True)
                for g in range(sub // 8):
                    tile = jnp.where(lane == o // 8 + g, mean[8 * g:8 * g + 8, :], tile)
                    tile = jnp.where(lane == 64 + o // 8 + g, m2[8 * g:8 * g + 8, :], tile)
            return tile

        def stats(tile0, row0, rows):
            lane = lanes()
            zero = jnp.zeros((8, 128), jnp.float32)
            if rows < _TILE:
                sbuf[tile0] = stats_unit(row0, rows, lane, zero)
                return

            def one_tile(t, carry):
                def unit(u, tile):
                    return stats_unit(row0 + t * _TILE + u * _UNIT, _UNIT,
                                      lane - u * (_UNIT // 8), tile)
                sbuf[tile0 + t] = lax.fori_loop(0, _TILE // _UNIT, unit, zero)
                return carry
            if rows == _TILE:
                one_tile(0, 0)
            else:
                lax.fori_loop(0, rows // _TILE, one_tile, 0)

        def merge(tile, direct):
            mine, theirs = sbuf[tile], rbuf[tile]
            s = mine + theirs
            delta = theirs - mine
            v = jnp.where(lanes() < 64, delta * delta * (N * N / n_total), s)
            if direct:
                return 0.5 * s, v * (1.0 / n_total)
            v = v + pltpu.roll(v, 64, 1)
            return 0.5 * s, lax.rsqrt(v * (1.0 / n_total) + _EPS)

        def norm_unit(row0, rows, lane, mean_t, scale_t, direct):
            for g in range(rows // 8):
                mask = lane == g
                mean = jnp.sum(jnp.where(mask, mean_t, 0.0), axis=1, keepdims=True)
                if direct:
                    var = jnp.sum(jnp.where((lane & 63) == g, scale_t, 0.0),
                                  axis=1, keepdims=True)
                    rstd = lax.rsqrt(var + _EPS)
                else:
                    rstd = jnp.sum(jnp.where(mask, scale_t, 0.0), axis=1, keepdims=True)
                r0 = pl.multiple_of(row0 + g * 8, 8)
                y = (xbuf[pl.ds(r0, 8), :] - mean) * rstd * gb8[0] + gb8[1]
                o_ref[pl.ds(r0, 8), :] = y.astype(o_ref.dtype)

        def normalize(tile0, row0, rows):
            lane = lanes()
            if rows < _TILE:
                direct = rows <= _DIRECT_MAX
                norm_unit(row0, rows, lane, *merge(tile0, direct), direct)
                return

            def one_tile(t, carry):
                mean_t, rstd_t = merge(tile0 + t, False)

                def unit(u, c):
                    norm_unit(row0 + t * _TILE + u * _UNIT, _UNIT,
                              lane - u * (_UNIT // 8), mean_t, rstd_t, False)
                    return c
                lax.fori_loop(0, _TILE // _UNIT, unit, 0)
                return carry
            if rows == _TILE:
                one_tile(0, 0)
            else:
                lax.fori_loop(0, rows // _TILE, one_tile, 0)

        def stream(big_sems, tail_sems, early_sems, gb_sem):
            def big_copy(b):
                rows = pl.ds(pl.multiple_of(b * _BIG, _BIG), _BIG)
                return pltpu.make_async_copy(x_hbm.at[rows], xbuf.at[rows], big_sems.at[b])

            def tail_copy(t):
                rows = pl.ds(tail_row[t], _TAIL[t])
                return pltpu.make_async_copy(x_hbm.at[rows], xbuf.at[rows], tail_sems.at[t])

            def tail_stat_copy(t):
                sem = (early_sems.at[n_big + early.index(t)] if t in early
                       else late_sems.at[late.index(t)])
                return stat_copy(tail_tile0[t], tail_tiles[t], sem)

            for b in range(n_big):
                big_copy(b).start(priority=1)
            for t in range(n_tail):
                tail_copy(t).start(priority=1)
            g_copy = pltpu.make_async_copy(g_hbm, gbuf, gb_sem)
            b_copy = pltpu.make_async_copy(b_hbm, bbuf, gb_sem)
            g_copy.start()
            b_copy.start()

            barrier = pltpu.get_barrier_semaphore()
            pl.semaphore_signal(barrier, inc=1, device_id=nbr,
                                device_id_type=pl.DeviceIdType.MESH)

            g_copy.wait()
            b_copy.wait()
            gb8[0] = jnp.broadcast_to(gbuf[...], (8, N))
            gb8[1] = jnp.broadcast_to(bbuf[...], (8, N))
            pl.semaphore_wait(barrier, 1)

            def big_block(b, carry):
                row0 = pl.multiple_of(b * _BIG, _BIG)
                big_copy(b).wait()
                stats(b * big_tiles, row0, _BIG)
                exchange = stat_copy(b * big_tiles, big_tiles, early_sems.at[b])
                exchange.start()
                exchange.wait_recv()
                normalize(b * big_tiles, row0, _BIG)
                return carry
            lax.fori_loop(0, n_big, big_block, 0)

            for t in range(n_tail):
                tail_copy(t).wait()
                stats(tail_tile0[t], tail_row[t], _TAIL[t])
                tail_stat_copy(t).start()
                if t < n_tail - 1:
                    for j in _NORM_AFTER[t]:
                        tail_stat_copy(j).wait_recv()
                        normalize(tail_tile0[j], tail_row[j], _TAIL[j])

        pl.run_scoped(
            stream,
            pltpu.SemaphoreType.DMA((n_big,)),
            pltpu.SemaphoreType.DMA((n_tail,)),
            pltpu.SemaphoreType.DMA((n_big + len(early),)),
            pltpu.SemaphoreType.DMA,
        )

        for i, t in enumerate(late):
            if i == len(late) - 1:
                pltpu.make_async_copy(sbuf, sbuf, send_sem).wait()
            stat_copy(tail_tile0[t], tail_tiles[t], late_sems.at[i]).wait_recv()
            normalize(tail_tile0[t], tail_row[t], _TAIL[t])

    return body, n_tiles, len(late)


def pallas_dist_layernorm_xy_m6144_n2048_kernel(
    x: jax.Array,
    gamma: jax.Array,
    beta: jax.Array,
):
    M, N = x.shape
    n_big = (M - sum(_TAIL)) // _BIG
    assert n_big >= 1 and n_big * _BIG + sum(_TAIL) == M
    body, n_tiles, n_late = _make_body(M, N, n_big)
    return pl.pallas_call(
        body,
        out_shape=pltpu.VMEM((M, N), jnp.bfloat16),
        in_specs=[pl.BlockSpec(memory_space=pltpu.HBM)] * 3,
        out_specs=pl.BlockSpec(memory_space=pltpu.VMEM),
        scratch_shapes=[
            pltpu.VMEM((M, N), jnp.float32),
            pltpu.VMEM((1, N), jnp.float32),
            pltpu.VMEM((1, N), jnp.float32),
            pltpu.VMEM((2, 8, N), jnp.float32),
            pltpu.VMEM((n_tiles, 8, 128), jnp.float32),
            pltpu.VMEM((n_tiles, 8, 128), jnp.float32),
            pltpu.SemaphoreType.DMA,
            pltpu.SemaphoreType.DMA((n_late,)),
        ],
        compiler_params=pltpu.CompilerParams(collective_id=0, vmem_limit_bytes=60 * 2**20),
    )(x, gamma.reshape(1, N), beta.reshape(1, N))
```

```python
import numpy as np

import jax
import jax.numpy as jnp
from jax import lax
from jax.experimental import pallas as pl
from jax.experimental.pallas import tpu as pltpu

_EPS = 1e-5
_Y_SIZE = 2
_BIG = 1024
_SWAP = 208
_SWAP_AT = 2
_TAIL = (512, 176, 96, 32)
_NORM_AFTER = ((), (), (), (0, 1, 2, 3))
_TILE = 512
_UNIT = 256
_SUB = 64
_DIRECT_MAX = 32


def _make_body(M, N, n_big):
    n_tail = len(_TAIL)
    assert all(r % 8 == 0 and (r < _TILE or r % _TILE == 0) for r in _TAIL) and _SWAP < _TILE
    n_total = _Y_SIZE * N
    swap_row = n_big * _BIG
    tail_row = [swap_row + _SWAP + int(s) for s in np.cumsum((0,) + _TAIL[:-1])]
    big_tiles = _BIG // _TILE
    tail_tiles = [-(-r // _TILE) for r in _TAIL]
    tail_tile0 = [n_big * big_tiles + int(s) for s in np.cumsum([0] + tail_tiles[:-1])]
    guest_tile = n_big * big_tiles + sum(tail_tiles)
    n_tiles = guest_tile + 1
    late = list(_NORM_AFTER[-1])
    early = [t for t in range(n_tail) if t not in late]
    assert sorted(early + late) == sorted(sum(map(list, _NORM_AFTER), []))

    def body(x_hbm, g_hbm, b_hbm, o_ref,
             xbuf, gbuf, bbuf, gb8, sbuf, rbuf, guest_x, guest_y,
             send_sem, late_sems, back_sems):
        nbr = (lax.axis_index("x"), 1 - lax.axis_index("y"))
        xnbr = (1 - lax.axis_index("x"), lax.axis_index("y"))

        def back_copy():
            return pltpu.make_async_remote_copy(
                src_ref=guest_y, dst_ref=o_ref.at[pl.ds(swap_row, _SWAP)],
                send_sem=back_sems.at[0], recv_sem=back_sems.at[1],
                device_id=xnbr, device_id_type=pl.DeviceIdType.MESH)

        def stat_copy(tile0, tiles, recv_sem):
            return pltpu.make_async_remote_copy(
                src_ref=sbuf.at[pl.ds(tile0, tiles)], dst_ref=rbuf.at[pl.ds(tile0, tiles)],
                send_sem=send_sem, recv_sem=recv_sem,
                device_id=nbr, device_id_type=pl.DeviceIdType.MESH)

        def lanes():
            return lax.broadcasted_iota(jnp.int32, (8, 128), 1)

        def stats_unit(src, row0, rows, lane, tile):
            for o in range(0, rows, _SUB):
                sub = min(_SUB, rows - o)
                r0 = pl.multiple_of(row0 + o, 8)
                mean = jnp.sum(src[pl.ds(r0, sub), :], axis=1, keepdims=True) * (1.0 / N)
                d = src[pl.ds(r0, sub), :] - mean
                m2 = jnp.sum(d * d, axis=1, keepdims=True)
                for g in range(sub // 8):
                    tile = jnp.where(lane == o // 8 + g, mean[8 * g:8 * g + 8, :], tile)
                    tile = jnp.where(lane == 64 + o // 8 + g, m2[8 * g:8 * g + 8, :], tile)
            return tile

        def stats(tile0, row0, rows, src=xbuf):
            lane = lanes()
            zero = jnp.zeros((8, 128), jnp.float32)
            if rows < _TILE:
                sbuf[tile0] = stats_unit(src, row0, rows, lane, zero)
                return

            def one_tile(t, carry):
                def unit(u, tile):
                    return stats_unit(src, row0 + t * _TILE + u * _UNIT, _UNIT,
                                      lane - u * (_UNIT // 8), tile)
                sbuf[tile0 + t] = lax.fori_loop(0, _TILE // _UNIT, unit, zero)
                return carry
            if rows == _TILE:
                one_tile(0, 0)
            else:
                lax.fori_loop(0, rows // _TILE, one_tile, 0)

        def merge(tile, direct):
            mine, theirs = sbuf[tile], rbuf[tile]
            s = mine + theirs
            delta = theirs - mine
            v = jnp.where(lanes() < 64, delta * delta * (N * N / n_total), s)
            if direct:
                return 0.5 * s, v * (1.0 / n_total)
            v = v + pltpu.roll(v, 64, 1)
            return 0.5 * s, lax.rsqrt(v * (1.0 / n_total) + _EPS)

        def norm_unit(src, dst, row0, rows, lane, mean_t, scale_t, direct):
            for g in range(rows // 8):
                mask = lane == g
                mean = jnp.sum(jnp.where(mask, mean_t, 0.0), axis=1, keepdims=True)
                if direct:
                    var = jnp.sum(jnp.where((lane & 63) == g, scale_t, 0.0),
                                  axis=1, keepdims=True)
                    rstd = lax.rsqrt(var + _EPS)
                else:
                    rstd = jnp.sum(jnp.where(mask, scale_t, 0.0), axis=1, keepdims=True)
                r0 = pl.multiple_of(row0 + g * 8, 8)
                y = (src[pl.ds(r0, 8), :] - mean) * rstd * gb8[0] + gb8[1]
                dst[pl.ds(r0, 8), :] = y.astype(dst.dtype)

        def normalize(tile0, row0, rows, src=xbuf, dst=o_ref):
            lane = lanes()
            if rows < _TILE:
                direct = rows <= _DIRECT_MAX
                norm_unit(src, dst, row0, rows, lane, *merge(tile0, direct), direct)
                return

            def one_tile(t, carry):
                mean_t, rstd_t = merge(tile0 + t, False)

                def unit(u, c):
                    norm_unit(src, dst, row0 + t * _TILE + u * _UNIT, _UNIT,
                              lane - u * (_UNIT // 8), mean_t, rstd_t, False)
                    return c
                lax.fori_loop(0, _TILE // _UNIT, unit, 0)
                return carry
            if rows == _TILE:
                one_tile(0, 0)
            else:
                lax.fori_loop(0, rows // _TILE, one_tile, 0)

        def stream(big_sems, tail_sems, early_sems, gb_sem, swap_sems):
            def big_copy(b):
                rows = pl.ds(pl.multiple_of(b * _BIG, _BIG), _BIG)
                return pltpu.make_async_copy(x_hbm.at[rows], xbuf.at[rows], big_sems.at[b])

            def tail_copy(t):
                rows = pl.ds(tail_row[t], _TAIL[t])
                return pltpu.make_async_copy(x_hbm.at[rows], xbuf.at[rows], tail_sems.at[t])

            def tail_stat_copy(t):
                sem = (early_sems.at[n_big + early.index(t)] if t in early
                       else late_sems.at[late.index(t)])
                return stat_copy(tail_tile0[t], tail_tiles[t], sem)

            for b in range(n_big):
                big_copy(b).start(priority=1)
            for t in range(n_tail):
                tail_copy(t).start(priority=1)
            g_copy = pltpu.make_async_copy(g_hbm, gbuf, gb_sem)
            b_copy = pltpu.make_async_copy(b_hbm, bbuf, gb_sem)
            g_copy.start()
            b_copy.start()

            barrier = pltpu.get_barrier_semaphore()
            for peer in (nbr, xnbr):
                pl.semaphore_signal(barrier, inc=1, device_id=peer,
                                    device_id_type=pl.DeviceIdType.MESH)
            pl.semaphore_wait(barrier, 2)

            lend = pltpu.make_async_remote_copy(
                src_ref=x_hbm.at[pl.ds(swap_row, _SWAP)], dst_ref=guest_x,
                send_sem=swap_sems.at[0], recv_sem=swap_sems.at[1],
                device_id=xnbr, device_id_type=pl.DeviceIdType.MESH)
            lend.start()

            g_copy.wait()
            b_copy.wait()
            gb8[0] = jnp.broadcast_to(gbuf[...], (8, N))
            gb8[1] = jnp.broadcast_to(bbuf[...], (8, N))

            def guest_block():
                lend.wait_recv()
                stats(guest_tile, 0, _SWAP, src=guest_x)
                exchange = stat_copy(guest_tile, 1, swap_sems.at[2])
                exchange.start()
                exchange.wait_recv()
                normalize(guest_tile, 0, _SWAP, src=guest_x, dst=guest_y)
                back_copy().start()
                lend.wait_send()

            def big_block(b, carry):
                row0 = pl.multiple_of(b * _BIG, _BIG)
                big_copy(b).wait()
                stats(b * big_tiles, row0, _BIG)
                exchange = stat_copy(b * big_tiles, big_tiles, early_sems.at[b])
                exchange.start()
                exchange.wait_recv()
                normalize(b * big_tiles, row0, _BIG)
                pl.when(b == min(_SWAP_AT, n_big - 1))(guest_block)
                return carry
            lax.fori_loop(0, n_big, big_block, 0)

            for t in range(n_tail):
                tail_copy(t).wait()
                stats(tail_tile0[t], tail_row[t], _TAIL[t])
                tail_stat_copy(t).start()
                if t < n_tail - 1:
                    for j in _NORM_AFTER[t]:
                        tail_stat_copy(j).wait_recv()
                        normalize(tail_tile0[j], tail_row[j], _TAIL[j])

        pl.run_scoped(
            stream,
            pltpu.SemaphoreType.DMA((n_big,)),
            pltpu.SemaphoreType.DMA((n_tail,)),
            pltpu.SemaphoreType.DMA((n_big + len(early),)),
            pltpu.SemaphoreType.DMA,
            pltpu.SemaphoreType.DMA((3,)),
        )

        for i, t in enumerate(late):
            if i == len(late) - 1:
                pltpu.make_async_copy(sbuf, sbuf, send_sem).wait()
                back_copy().wait()
            stat_copy(tail_tile0[t], tail_tiles[t], late_sems.at[i]).wait_recv()
            normalize(tail_tile0[t], tail_row[t], _TAIL[t])

    return body, n_tiles, len(late)


def pallas_dist_layernorm_xy_m6144_n2048_kernel(
    x: jax.Array,
    gamma: jax.Array,
    beta: jax.Array,
):
    M, N = x.shape
    n_big = (M - sum(_TAIL) - _SWAP) // _BIG
    assert n_big >= 1 and n_big * _BIG + _SWAP + sum(_TAIL) == M
    body, n_tiles, n_late = _make_body(M, N, n_big)
    return pl.pallas_call(
        body,
        out_shape=pltpu.VMEM((M, N), jnp.bfloat16),
        in_specs=[pl.BlockSpec(memory_space=pltpu.HBM)] * 3,
        out_specs=pl.BlockSpec(memory_space=pltpu.VMEM),
        scratch_shapes=[
            pltpu.VMEM((M, N), jnp.float32),
            pltpu.VMEM((1, N), jnp.float32),
            pltpu.VMEM((1, N), jnp.float32),
            pltpu.VMEM((2, 8, N), jnp.float32),
            pltpu.VMEM((n_tiles, 8, 128), jnp.float32),
            pltpu.VMEM((n_tiles, 8, 128), jnp.float32),
            pltpu.VMEM((_SWAP, N), jnp.float32),
            pltpu.VMEM((_SWAP, N), jnp.bfloat16),
            pltpu.SemaphoreType.DMA,
            pltpu.SemaphoreType.DMA((n_late,)),
            pltpu.SemaphoreType.DMA((2,)),
        ],
        compiler_params=pltpu.CompilerParams(collective_id=0, vmem_limit_bytes=60 * 2**20),
    )(x, gamma.reshape(1, N), beta.reshape(1, N))
```
